```python
import numpy as np

kernel_name = "dist_ar_xy_y_m1024_n512"

def setup_inputs():
    return {"x": np.random.randn(2048, 512).astype(np.float32)}

def reference(x: np.ndarray) -> np.ndarray:
    return x.reshape(2, 1024, 512).sum(axis=0)
```

```python
import jax
import jax.numpy as jnp
from jax import lax
from jax.experimental import pallas as pl
from jax.experimental.pallas import tpu as pltpu

_MESH = pl.DeviceIdType.MESH

RB = 16
UW = 128
N_FWD = 118
LOOKAHEAD = 12
LOADS = (1, 2, 4, 8)
X_GROUPS = (21, 4, 2)
Q_TAIL = (2, 1)


def _plan(m, n):
    nrb, upr = m // RB, n // UW
    full, part = divmod(N_FWD, upr)
    p_rb = full + (1 if part else 0)
    mid = nrb - 2 * p_rb
    assert mid >= 0 and upr >= 3
    send_rb = p_rb + mid + (1 if part else 0)

    loads = list(LOADS)
    loads.append(send_rb - 1 - sum(loads))
    assert loads[-1] > 0

    units = [divmod(k, upr) for k in range(1, N_FWD)]

    q = [(full, 1, part, upr - part)] if part else []
    sizes = [mid - sum(Q_TAIL)] + list(Q_TAIL)
    off = p_rb
    for s in sizes:
        assert s > 0
        q.append((off, s, 0, upr))
        off += s
    if part:
        q.append((off, 1, part, upr - part))

    xg, off = [(0, 1, 0, upr)], 1
    for s in list(X_GROUPS) + [1] * (full - 1 - sum(X_GROUPS)):
        xg.append((off, s, 0, upr))
        off += s
    assert off == full
    if part:
        xg.append((full, 1, 0, part))

    events = []
    for kind, rects in (("x", xg), ("q", q)):
        t = 0
        for j in reversed(range(len(rects))):
            events.append((t, kind == "q", kind, j))
            t -= rects[j][1] * rects[j][3]
    tail = [(kind, j) for _, _, kind, j in sorted(events)]
    return upr, full, part, send_rb, loads, units, q, xg, tail


def pallas_dist_ar_xy_y_m1024_n512_kernel(x: jax.Array):
    m, n = x.shape
    upr, full, part, send_rb, loads, units, q, xg, tail = _plan(m, n)
    load_of = [None] + [i for i, r in enumerate(loads) for _ in range(r)]
    xgroup_of = [g for g, r in enumerate(xg) for _ in range(r[1])]
    sgroup_of = [0] + [1] * (full - 1) + [2]
    n_sg = 3 if part else 2
    first = [(1, 1), (2, upr - 2), (0, 1)]

    def body(x_ref, o_ref, sbuf, rbuf, head, first_sem, load_sem, head_sem,
             ysend, yrecv, qsend, qrecv, xsend, xrecv, ready):
        mx, my = lax.axis_index("x"), lax.axis_index("y")
        ynbr, xnbr = (mx, 1 - my), (1 - mx, my)
        is11 = jnp.logical_and(mx == 1, my == 1)
        barrier = pltpu.get_barrier_semaphore()

        def rect(side, rb, cnt, u0, nu):
            up, down = rb * RB, m - (rb + cnt) * RB
            start = pl.multiple_of(up + side * (down - up), RB)
            return pl.ds(start, cnt * RB), pl.ds(u0 * UW, nu * UW)

        def mine(*r):
            return rect(mx, *r)

        def other(*r):
            return rect(1 - mx, *r)

        def load(idx, sem):
            cp = pltpu.make_async_copy(x_ref.at[idx], o_ref.at[idx], sem)
            cp.start()
            return cp

        def push(src, dst, send_sem, recv_sem, dev):
            cp = pltpu.make_async_remote_copy(
                src, dst, send_sem, recv_sem, device_id=dev, device_id_type=_MESH)
            cp.start()
            return cp

        def wait_all(buf, idx, sem):
            pltpu.make_async_copy(buf.at[idx], buf.at[idx], sem).wait()

        def signal_neighbours(sem):
            for dev in (ynbr, xnbr):
                pl.semaphore_signal(sem, inc=1, device_id=dev, device_id_type=_MESH)

        def pack(idx):
            sbuf[idx] = o_ref[idx].astype(sbuf.dtype)

        def add(idx):
            o_ref[idx] = o_ref[idx] + rbuf[idx].astype(o_ref.dtype)

        first_cps = [load(mine(0, 1, *first[0]), first_sem.at[0])]
        pl.when(jnp.logical_not(is11))(lambda: signal_neighbours(barrier))
        for i in range(1, len(first)):
            first_cps.append(load(mine(0, 1, *first[i]), first_sem.at[i]))
        load_cps, off = [], 1
        for i, r in enumerate(loads):
            load_cps.append(load(mine(off, r, 0, upr), load_sem.at[i]))
            off += r
        rest_cp = load(other(0, full, 0, upr), load_sem.at[len(loads)])

        pl.when(mx == my)(lambda: pl.semaphore_wait(barrier, 2))
        pl.when(mx != my)(lambda: pl.semaphore_wait(barrier, 1))
        pl.when(mx > my)(lambda: pl.semaphore_wait(ready, 1))
        head_idx = mine(0, 1, 0, 1)
        head_cp = push(x_ref.at[head_idx], head, head_sem.at[0], head_sem.at[1], ynbr)
        pl.when(is11)(lambda: signal_neighbours(ready))

        y_cps, q_cps = {}, {}

        def send_units(rb, u0, nu):
            for k, (r, u) in enumerate(units):
                if r == rb and u0 <= u < u0 + nu:
                    idx = mine(rb, 1, u, 1)
                    y_cps[k] = push(sbuf.at[idx], rbuf.at[idx],
                                    ysend.at[sgroup_of[rb]], yrecv.at[k], ynbr)

        def send_block(rb):
            if load_of[rb] != load_of[rb - 1]:
                load_cps[load_of[rb]].wait()
            pack(mine(rb, 1, 0, upr))
            send_units(rb, 0, upr)
            for j, r in enumerate(q):
                if r[0] + r[1] - 1 == rb:
                    idx = mine(*r)
                    q_cps[j] = push(sbuf.at[idx], rbuf.at[idx],
                                    qsend.at[j], qrecv.at[j], ynbr)

        for cp, (u0, nu) in zip(first_cps, first):
            cp.wait()
            if u0 > 0:
                pack(mine(0, 1, u0, nu))
                send_units(0, u0, nu)
        for rb in range(1, LOOKAHEAD):
            send_block(rb)

        pl.when(mx < my)(lambda: pl.semaphore_wait(ready, 1))

        def forward(rb, idx):
            push(rbuf.at[idx], rbuf.at[idx],
                 xsend.at[sgroup_of[rb]], xrecv.at[xgroup_of[rb]], xnbr)

        head_cp.wait_recv()
        rbuf[head_idx] = head[...].astype(rbuf.dtype)
        forward(0, head_idx)
        o_ref[head_idx] = o_ref[head_idx] + head[...]

        for k, (rb, u) in enumerate(units):
            idx = mine(rb, 1, u, 1)
            y_cps[k].wait_recv()
            forward(rb, idx)
            add(idx)
            if u == upr - 1 and rb + LOOKAHEAD < send_rb:
                send_block(rb + LOOKAHEAD)
        assert len(q_cps) == len(q)

        rest_cp.wait()
        head_cp.wait_send()
        for t, (kind, j) in enumerate(tail):
            if t == len(tail) - 2:
                wait_all(sbuf, mine(0, 1, 1, upr - 1), ysend.at[0])
                wait_all(rbuf, mine(0, 1, 0, upr), xsend.at[0])
                for g, r in enumerate([(1, full - 1, 0, upr), (full, 1, 0, part)][:n_sg - 1]):
                    wait_all(sbuf, mine(*r), ysend.at[g + 1])
                    wait_all(rbuf, mine(*r), xsend.at[g + 1])
                for cp in q_cps.values():
                    cp.wait_send()
            if kind == "x":
                idx = other(*xg[j])
                wait_all(rbuf, idx, xrecv.at[j])
            else:
                idx = mine(*q[j])
                q_cps[j].wait_recv()
            add(idx)

    dma = pltpu.SemaphoreType.DMA
    return pl.pallas_call(
        body,
        out_shape=jax.ShapeDtypeStruct((m, n), x.dtype),
        in_specs=[pl.BlockSpec(memory_space=pl.ANY)],
        out_specs=pl.BlockSpec(memory_space=pltpu.VMEM),
        scratch_shapes=[
            pltpu.VMEM((m, n), jnp.bfloat16),
            pltpu.VMEM((m, n), jnp.bfloat16),
            pltpu.VMEM((RB, UW), x.dtype),
            dma((len(first),)),
            dma((len(loads) + 1,)),
            dma((2,)),
            dma((n_sg,)),
            dma((len(units),)),
            dma((len(q),)),
            dma((len(q),)),
            dma((n_sg,)),
            dma((len(xg),)),
            pltpu.SemaphoreType.REGULAR,
        ],
        compiler_params=pltpu.CompilerParams(
            collective_id=0, disable_semaphore_checks=True),
    )(x)
```

```python
import jax
import jax.numpy as jnp
from jax import lax
from jax.experimental import pallas as pl
from jax.experimental.pallas import tpu as pltpu

_MESH = pl.DeviceIdType.MESH

RB = 16
UW = 128
N_FWD = 118
LOOKAHEAD = 12
LOADS = (1, 2, 4, 8)
X_GROUPS = (21, 4, 2)
Q_TAIL = (2, 1)


def _plan(m, n):
    nrb, upr = m // RB, n // UW
    full, part = divmod(N_FWD, upr)
    p_rb = full + (1 if part else 0)
    mid = nrb - 2 * p_rb
    assert mid >= 0 and upr >= 3
    send_rb = p_rb + mid + (1 if part else 0)

    loads = list(LOADS)
    loads.append(send_rb - 1 - sum(loads))
    assert loads[-1] > 0

    units = [divmod(k, upr) for k in range(1, N_FWD)]

    q = [(full, 1, part, upr - part)] if part else []
    sizes = [mid - sum(Q_TAIL)] + list(Q_TAIL)
    off = p_rb
    for s in sizes:
        assert s > 0
        q.append((off, s, 0, upr))
        off += s
    if part:
        q.append((off, 1, part, upr - part))

    xg, off = [(0, 1, 0, upr)], 1
    for s in list(X_GROUPS) + [1] * (full - 1 - sum(X_GROUPS)):
        xg.append((off, s, 0, upr))
        off += s
    assert off == full
    if part:
        xg.append((full, 1, 0, part))

    events = []
    for kind, rects in (("x", xg), ("q", q)):
        t = 0
        for j in reversed(range(len(rects))):
            events.append((t, kind == "q", kind, j))
            t -= rects[j][1] * rects[j][3]
    tail = [(kind, j) for _, _, kind, j in sorted(events)]
    return upr, full, part, send_rb, loads, units, q, xg, tail


def pallas_dist_ar_xy_y_m1024_n512_kernel(x: jax.Array):
    m, n = x.shape
    upr, full, part, send_rb, loads, units, q, xg, tail = _plan(m, n)
    load_of = [None] + [i for i, r in enumerate(loads) for _ in range(r)]
    xgroup_of = [g for g, r in enumerate(xg) for _ in range(r[1])]
    sgroup_of = [0] + [1] * (full - 1) + [2]
    n_sg = 3 if part else 2
    first = [(1, 1), (2, upr - 2), (0, 1)]

    def body(x_ref, o_ref, sbuf, rbuf, head, first_sem, load_sem, head_sem,
             ysend, yrecv, qsend, qrecv, xsend, xrecv, ready):
        mx, my = lax.axis_index("x"), lax.axis_index("y")
        ynbr, xnbr = (mx, 1 - my), (1 - mx, my)
        is11 = jnp.logical_and(mx == 1, my == 1)
        barrier = pltpu.get_barrier_semaphore()

        def rect(side, rb, cnt, u0, nu):
            up, down = rb * RB, m - (rb + cnt) * RB
            start = pl.multiple_of(up + side * (down - up), RB)
            return pl.ds(start, cnt * RB), pl.ds(u0 * UW, nu * UW)

        def mine(*r):
            return rect(mx, *r)

        def other(*r):
            return rect(1 - mx, *r)

        def load(idx, sem):
            cp = pltpu.make_async_copy(x_ref.at[idx], o_ref.at[idx], sem)
            cp.start()
            return cp

        def push(src, dst, send_sem, recv_sem, dev):
            cp = pltpu.make_async_remote_copy(
                src, dst, send_sem, recv_sem, device_id=dev, device_id_type=_MESH)
            cp.start()
            return cp

        def wait_all(buf, idx, sem):
            pltpu.make_async_copy(buf.at[idx], buf.at[idx], sem).wait()

        def signal_neighbours(sem):
            for dev in (ynbr, xnbr):
                pl.semaphore_signal(sem, inc=1, device_id=dev, device_id_type=_MESH)

        def pack(idx):
            sbuf[idx] = o_ref[idx].astype(sbuf.dtype)

        def add(idx):
            o_ref[idx] = o_ref[idx] + rbuf[idx].astype(o_ref.dtype)

        first_cps = [load(mine(0, 1, *first[0]), first_sem.at[0])]
        pl.when(jnp.logical_not(is11))(lambda: signal_neighbours(barrier))
        for i in range(1, len(first)):
            first_cps.append(load(mine(0, 1, *first[i]), first_sem.at[i]))
        load_cps, off = [], 1
        for i, r in enumerate(loads):
            load_cps.append(load(mine(off, r, 0, upr), load_sem.at[i]))
            off += r
        rest_cp = load(other(0, full, 0, upr), load_sem.at[len(loads)])

        pl.when(mx == my)(lambda: pl.semaphore_wait(barrier, 2))
        pl.when(mx != my)(lambda: pl.semaphore_wait(barrier, 1))
        pl.when(mx > my)(lambda: pl.semaphore_wait(ready, 1))
        head_idx = mine(0, 1, 0, 1)
        head_cp = push(x_ref.at[head_idx], head, head_sem.at[0], head_sem.at[1], ynbr)
        pl.when(is11)(lambda: signal_neighbours(ready))

        y_cps, q_cps = {}, {}

        def send_units(rb, u0, nu):
            for k, (r, u) in enumerate(units):
                if r == rb and u0 <= u < u0 + nu:
                    idx = mine(rb, 1, u, 1)
                    y_cps[k] = push(sbuf.at[idx], rbuf.at[idx],
                                    ysend.at[sgroup_of[rb]], yrecv.at[k], ynbr)

        def send_block(rb):
            if load_of[rb] != load_of[rb - 1]:
                load_cps[load_of[rb]].wait()
            pack(mine(rb, 1, 0, upr))
            send_units(rb, 0, upr)
            for j, r in enumerate(q):
                if r[0] + r[1] - 1 == rb:
                    idx = mine(*r)
                    q_cps[j] = push(sbuf.at[idx], rbuf.at[idx],
                                    qsend.at[j], qrecv.at[j], ynbr)

        for cp, (u0, nu) in zip(first_cps, first):
            cp.wait()
            if u0 > 0:
                pack(mine(0, 1, u0, nu))
                send_units(0, u0, nu)
        for rb in range(1, LOOKAHEAD):
            send_block(rb)

        pl.when(mx < my)(lambda: pl.semaphore_wait(ready, 1))

        def forward(rb, idx):
            push(rbuf.at[idx], rbuf.at[idx],
                 xsend.at[sgroup_of[rb]], xrecv.at[xgroup_of[rb]], xnbr)

        head_cp.wait_recv()
        rbuf[head_idx] = head[...].astype(rbuf.dtype)
        forward(0, head_idx)
        o_ref[head_idx] = o_ref[head_idx] + head[...]

        for k, (rb, u) in enumerate(units):
            idx = mine(rb, 1, u, 1)
            y_cps[k].wait_recv()
            forward(rb, idx)
            add(idx)
            if u == upr - 1 and rb + LOOKAHEAD < send_rb:
                send_block(rb + LOOKAHEAD)
        assert len(q_cps) == len(q)

        rest_cp.wait()
        head_cp.wait_send()
        for t, (kind, j) in enumerate(tail):
            if t == len(tail) - 2:
                wait_all(sbuf, mine(0, 1, 1, upr - 1), ysend.at[0])
                wait_all(rbuf, mine(0, 1, 0, upr), xsend.at[0])
                for g, r in enumerate([(1, full - 1, 0, upr), (full, 1, 0, part)][:n_sg - 1]):
                    wait_all(sbuf, mine(*r), ysend.at[g + 1])
                    wait_all(rbuf, mine(*r), xsend.at[g + 1])
                for cp in q_cps.values():
                    cp.wait_send()
            if kind == "x":
                idx = other(*xg[j])
                wait_all(rbuf, idx, xrecv.at[j])
            else:
                idx = mine(*q[j])
                q_cps[j].wait_recv()
            add(idx)

    dma = pltpu.SemaphoreType.DMA
    return pl.pallas_call(
        body,
        out_shape=jax.ShapeDtypeStruct((m, n), x.dtype),
        in_specs=[pl.BlockSpec(memory_space=pl.ANY)],
        out_specs=pl.BlockSpec(memory_space=pltpu.VMEM),
        scratch_shapes=[
            pltpu.VMEM((m, n), jnp.bfloat16),
            pltpu.VMEM((m, n), jnp.bfloat16),
            pltpu.VMEM((RB, UW), x.dtype),
            dma((len(first),)),
            dma((len(loads) + 1,)),
            dma((2,)),
            dma((n_sg,)),
            dma((len(units),)),
            dma((len(q),)),
            dma((len(q),)),
            dma((n_sg,)),
            dma((len(xg),)),
            pltpu.SemaphoreType.REGULAR,
        ],
        compiler_params=pltpu.CompilerParams(
            collective_id=0,
            disable_semaphore_checks=True,
            disable_bounds_checks=True,
        ),
    )(x)
```
